```python
import numpy as np

kernel_name = "dist_sparse_attn_strided_kvseq_b1_sq256_skv4096_hq8_dh128"

def setup_inputs():
    x = np.random.randn(1, 256, 1024).astype(np.float32)
    Wq = np.random.randn(1024, 1024).astype(np.float32) * 0.02
    K_ext = np.random.randn(1, 16384, 8, 128).astype(np.float32)
    V_ext = np.random.randn(1, 16384, 8, 128).astype(np.float32)
    Wo = np.random.randn(1024, 1024).astype(np.float32) * 0.02
    return {"x": x, "Wq": Wq, "K_ext": K_ext, "V_ext": V_ext, "Wo": Wo}

def reference(x, Wq, K_ext, V_ext, Wo):
    B, Sq, Skv, Hq, Dh = 1, 256, 16384, 8, 128
    Q = (x @ Wq).reshape(B, Sq, Hq, Dh)
    qb = (np.arange(Sq) // 64)[:, None]
    kb = (np.arange(Skv) // 64)[None, :]
    mask = (qb == kb) | ((kb % 4) == (qb % 4))
    scores = np.einsum('bihd,bjhd->bhij', Q, K_ext).astype(np.float32) * 0.08838834764831843
    scores = np.where(mask[None, None, :, :], scores, -1e9)
    scores_max = scores.max(axis=-1, keepdims=True)
    w = np.exp(scores - scores_max)
    row_keep = mask.any(axis=1)
    w_sum = np.where(row_keep[None, None, :, None], w.sum(axis=-1, keepdims=True), 1.0)
    w = w / w_sum
    w = np.where(row_keep[None, None, :, None], w, 0.0)
    ctx = np.einsum('bhij,bjhd->bihd', w, V_ext).reshape(B, Sq, Hq * Dh)
    return ctx @ Wo
```

```python
import contextlib
import math

import jax
import jax.numpy as jnp
from jax import lax
from jax.experimental import pallas as pl
from jax.experimental.pallas import tpu as pltpu

SQ, DM, HEADS, DH = 256, 1024, 8, 128
BLK = 64
NQB = SQ // BLK
KBLKS = 16
NPIECE = NQB * HEADS
LAST = NPIECE - 1
Q_SCALE = 0.08838834764831843 * math.log2(math.e)
F32, BF16 = jnp.float32, jnp.bfloat16
MESH = pl.DeviceIdType.MESH


def make(n_root=6, window=10, root_lag=1, merge_root=(29,), merge_rest=(31,), mid_root=30, fwd_at=(15, 19, 23, 28), scope=False, prio=False,
         checks=False, left=512):
    n_mid = HEADS - 1 - n_root
    root_pieces = NQB * n_root
    tail_piece = NPIECE - NQB
    tail_group = NQB + n_mid
    n_group = tail_group + 2

    def sc(name):
        return jax.named_scope("s_" + name) if scope else contextlib.nullcontext()

    def body(x_hbm, wq_hbm, k_hbm, v_hbm, wo_hbm, out_ref,
             kbuf, vbuf, x_f32, wq_f32, wo_f32, x_bf, wq_bf, q_bf,
             part, stats, ctx_mid, root_out, acc,
             k_sem, v_sem, w_sem, wo_sem,
             x_recv, q_recv, part_recv, stat_recv, out_recv,
             x_send, q_send, part_send, stat_send, out_send):

        def coords(p):
            if isinstance(p, int):
                return p // n_root, p % n_root
            r = p - root_pieces
            is_root = p < root_pieces
            return (jnp.where(is_root, lax.div(p, n_root), r & (NQB - 1)),
                    jnp.where(is_root, lax.rem(p, n_root), n_root + (r >> 2)))

        def k_copy(p):
            b, h = coords(p)
            return pltpu.make_async_copy(k_hbm.at[:, b, :, h, :], kbuf.at[p], k_sem.at[p])

        def v_copy(p):
            b, h = coords(p)
            return pltpu.make_async_copy(v_hbm.at[:, b, :, h, :], vbuf.at[p], v_sem.at[p])

        def wo_copy(h0, n, cols, sem):
            idx = (pl.ds(h0 * DH, n * DH), cols)
            return pltpu.make_async_copy(wo_hbm.at[idx], wo_f32.at[idx], wo_sem.at[sem])

        wo_early = lambda: wo_copy(0, HEADS - 1, slice(None), 0)
        wo_middle = lambda: wo_copy(n_root, n_mid, slice(None), 0)
        wo_left = lambda: wo_copy(HEADS - 1, 1, pl.ds(0, left), 1)
        wo_right = lambda: wo_copy(HEADS - 1, 1, pl.ds(left, DM - left), 2)

        def x_copy(b):
            return pltpu.make_async_copy(x_hbm.at[b], x_f32.at[b], w_sem.at[b])

        def wait_for(ref, sem):
            pltpu.make_async_copy(ref, ref, sem).wait()

        def send(src, dst, send_sem, recv_sem, peer):
            pltpu.make_async_remote_copy(src, dst, send_sem, recv_sem, device_id=(peer,),
                                         device_id_type=MESH).start()

        vprio = 1 if prio else 0
        k_copy(0).start()
        me = lax.axis_index("i")
        is_root_chip = me == 0
        not_root_chip = me != 0
        is_x_chip = me == 2
        is_q_chip = (me & 1) == 1
        half = me >> 1
        hop0 = jnp.where(is_root_chip, 2, me)
        hop1 = jnp.where(hop0 == 3, 1, hop0 + 1)
        hop2 = 6 - hop0 - hop1

        @pl.when(is_root_chip)
        def _():
            wo_early().start()

        @pl.when(is_x_chip)
        def _():
            for b in range(NQB):
                x_copy(b).start()

        @pl.when(is_q_chip)
        def _():
            cols = pl.ds(pl.multiple_of(half * (DM // 2), DM // 2), DM // 2)
            pltpu.make_async_copy(wq_hbm.at[:, cols], wq_f32, w_sem.at[0]).start()

        barrier = pltpu.get_barrier_semaphore()
        for j in (1, 2, 3):
            pl.semaphore_signal(barrier, inc=1, device_id=(me ^ j,), device_id_type=MESH)

        v_copy(0).start(priority=vprio)

        @pl.loop(1, window)
        def _(p):
            k_copy(p).start()
            v_copy(p).start(priority=vprio)

        pl.semaphore_wait(barrier, 3)

        with sc("weights"):
            @pl.when(is_x_chip)
            def _():
                @pl.loop(0, NQB)
                def _(b):
                    x_copy(b).wait()
                    x_bf[b] = x_f32[b].astype(BF16)
                    for j in (1, 3):
                        send(x_bf.at[b], x_bf.at[b], x_send, x_recv.at[b], me ^ j)

            @pl.when(is_q_chip)
            def _():
                wait_for(wq_f32, w_sem.at[0])

                @pl.loop(0, DM // DH)
                def _(c):
                    rows = pl.ds(pl.multiple_of(c * DH, DH), DH)
                    wq_bf[rows, :] = wq_f32[rows, :].astype(BF16)

            @pl.when(is_root_chip)
            def _():
                wo_early().wait()

        def project_q(b):
            wait_for(x_bf.at[b], x_recv.at[b])
            q = jnp.dot(x_bf[b], wq_bf[...], preferred_element_type=F32) * Q_SCALE
            q = q.astype(BF16)
            for i in range(HEADS // 2):
                q_bf[b, half, i] = q[:, i * DH:(i + 1) * DH]
            for j in (2, 1, 3):
                send(q_bf.at[b, half], q_bf.at[b, half], q_send, q_recv.at[b], me ^ j)

        def merge_weights(g):
            wait_for(stats.at[g, pl.ds(1, 3)], stat_recv.at[g])
            st = [stats[g, j] for j in range(4)]
            sw = [pltpu.roll(s, BLK, 1) for s in st]
            low = lax.broadcasted_iota(jnp.int32, (8, DH), 1) < BLK
            m = [jnp.where(low, a, b) for a, b in zip(st, sw)]
            l = [jnp.where(low, b, a) for a, b in zip(st, sw)]
            top = jnp.maximum(jnp.maximum(m[0], m[1]), jnp.maximum(m[2], m[3]))
            e = [jnp.exp2(mj - top) for mj in m]
            inv = 1.0 / (e[0] * l[0] + e[1] * l[1] + e[2] * l[2] + e[3] * l[3])
            return [jnp.where(low, e[j], e[j + 1]) * inv for j in (0, 2)]

        def expand(pairs, slot):
            out = []
            for pair in pairs:
                cols = jnp.broadcast_to(pair[slot:slot + 1], (DH, DH)).T
                out += [cols[:BLK], cols[BLK:]]
            return out

        def merge(p, w):
            t = [part[p, j].astype(F32) * w[j] for j in range(4)]
            return ((t[0] + t[1]) + (t[2] + t[3])).astype(BF16)

        def merge_group(g, p0, n):
            pairs = merge_weights(g)
            wait_for(part.at[pl.ds(p0, n), pl.ds(1, 3)], part_recv.at[g])
            return [merge(p0 + i, expand(pairs, i)) for i in range(n)]

        def project_root(b):
            c = jnp.concatenate(merge_group(b, b * n_root, n_root), axis=1)
            res = jnp.dot(c, wo_f32[pl.ds(0, n_root * DH), :].astype(BF16), preferred_element_type=F32)
            root_out[b] = res.astype(BF16).reshape(2, BLK // 2, DM)
            for j in (1, 3):
                send(root_out.at[b], root_out.at[b], out_send, out_recv.at[b], j)

        def forward(b):
            wait_for(root_out.at[b], out_recv.at[b])
            send(root_out.at[b, half], root_out.at[b, half], out_send, out_recv.at[b], 2)

        def piece(p, packed):
            b, h = coords(p)
            is_root = p < root_pieces
            at_end = p == LAST
            g = jnp.where(is_root, b, jnp.where(at_end, tail_group + 1, h + (NQB - n_root)))
            slot = jnp.where(is_root, h, b)
            closes_group = jnp.logical_or(slot == jnp.where(is_root, n_root - 1, NQB - 1), p == LAST - 1)

            @pl.when(h == 0)
            def _():
                with sc("q"):
                    @pl.when(is_q_chip)
                    def _():
                        @pl.loop(jnp.where(b == 0, 0, b + 1), jnp.minimum(b + 2, NQB))
                        def _(bq):
                            project_q(bq)
                        wait_for(q_bf.at[b, 1 - half], q_recv.at[b])

                    @pl.when(jnp.logical_not(is_q_chip))
                    def _():
                        wait_for(q_bf.at[b], q_recv.at[b])

            @pl.when(p + window < NPIECE)
            def _():
                k_copy(p + window).start()
                v_copy(p + window).start(priority=vprio)

            @pl.when(p + window == NPIECE)
            def _():
                @pl.when(not_root_chip)
                def _():
                    wo_middle().start()
                wo_left().start()
                wo_right().start()

            def share(buf, i, send_sem, recv_sem):
                @pl.when(jnp.logical_or(not_root_chip, jnp.logical_not(is_root)))
                def _():
                    send(buf.at[i, 0], buf.at[i, hop0], send_sem, recv_sem.at[g], me ^ hop0)

                @pl.when(jnp.logical_not(is_root))
                def _():
                    for j in (hop1, hop2):
                        send(buf.at[i, 0], buf.at[i, j], send_sem, recv_sem.at[g], me ^ j)

            with sc("piece"):
                k_copy(p).wait()
                q = q_bf[b, h >> 2, h & 3]
                k = kbuf[p].reshape(KBLKS * BLK, DH).astype(BF16)
                s = lax.dot_general(q, k, (((1,), (1,)), ((), ())), preferred_element_type=F32)
                m = jnp.max(s, axis=1, keepdims=True)
                e = jnp.exp2(s - m)
                l = jnp.sum(e, axis=1, keepdims=True)
                shift = (lax.broadcasted_iota(jnp.int32, (BLK, DH), 1)
                         - lax.broadcasted_iota(jnp.int32, (BLK, DH), 0))
                diag = jnp.where(shift == 0, m, jnp.where(shift == BLK, l, 0.0))
                row = jnp.sum(diag, axis=0, keepdims=True)
                packed = jnp.where(lax.broadcasted_iota(jnp.int32, (8, DH), 0) == slot, row, packed)
                e = e.astype(BF16)

                @pl.when(closes_group)
                def _():
                    stats[g, 0] = packed
                    share(stats, g, stat_send, stat_recv)

                v_copy(p).wait()
                v = vbuf[p].reshape(KBLKS * BLK, DH).astype(BF16)
                part[p, 0] = jnp.dot(e, v, preferred_element_type=F32).astype(BF16)
                share(part, p, part_send, part_recv)

            done = p + 1 - root_lag

            @pl.when(is_root_chip & (done > 0) & (done <= root_pieces) & (lax.rem(done, n_root) == 0))
            def _():
                with sc("root"):
                    project_root(lax.div(done, n_root) - 1)

            fwd = sum(jnp.where(p == at, i + 1, 0) for i, at in enumerate(fwd_at))

            @pl.when(jnp.logical_and(is_q_chip, fwd > 0))
            def _():
                with sc("fwd"):
                    forward(fwd - 1)

            mid = sum(jnp.where(p == jnp.where(is_root_chip, a, c), i + 1, 0)
                      for i, (a, c) in enumerate(zip(merge_root, merge_rest)))

            @pl.when(mid > 0)
            def _():
                with sc("merge"):
                    r = mid - 1
                    ctx_mid[r] = jnp.concatenate(merge_group(NQB + r, root_pieces + r * NQB, NQB), axis=0)

            @pl.when(p == jnp.where(is_root_chip, mid_root, LAST))
            def _():
                with sc("mid"):
                    @pl.when(is_x_chip)
                    def _():
                        for i in range(NQB):
                            wait_for(root_out.at[i], out_recv.at[i])

                    @pl.when(not_root_chip)
                    def _():
                        wo_middle().wait()

                    c = jnp.concatenate([ctx_mid[r] for r in range(n_mid)], axis=1)
                    w = wo_f32[pl.ds(n_root * DH, n_mid * DH), :].astype(BF16)
                    acc[...] = root_out[...].reshape(SQ, DM).astype(F32) + jnp.dot(c, w, preferred_element_type=F32)

            return packed

        lax.fori_loop(0, NPIECE, piece, jnp.ones((8, DH), F32))

        lc, rc = pl.ds(0, left), pl.ds(left, DM - left)
        top, bottom = pl.ds(0, SQ - BLK), pl.ds(SQ - BLK, BLK)
        last_rows = pl.ds(DM - DH, DH)
        with sc("merge7"):
            head = jnp.concatenate(merge_group(tail_group, tail_piece, NQB - 1), axis=0)
        with sc("left"):
            wo_left().wait()
            w = expand(merge_weights(tail_group + 1), NQB - 1)
            wl = wo_f32[last_rows, lc].astype(BF16)
            out_ref[top, lc] = (acc[top, lc] + jnp.dot(head, wl, preferred_element_type=F32)).astype(BF16)
        with sc("right"):
            wo_right().wait()
            wait_for(part.at[LAST, pl.ds(1, 3)], part_recv.at[tail_group + 1])
            tail = merge(LAST, w)
            wr = wo_f32[last_rows, rc].astype(BF16)
            full = jnp.concatenate([head, tail], axis=0)
            out_ref[:, rc] = (acc[:, rc] + jnp.dot(full, wr, preferred_element_type=F32)).astype(BF16)
            out_ref[bottom, lc] = (acc[bottom, lc] + jnp.dot(tail, wl, preferred_element_type=F32)).astype(BF16)

        with sc("drain"):
            wait_for(part.at[pl.ds(root_pieces, NPIECE - root_pieces), pl.ds(1, 3)], part_send)
            wait_for(stats.at[pl.ds(NQB, n_group - NQB), pl.ds(1, 3)], stat_send)

            @pl.when(not_root_chip)
            def _():
                wait_for(part.at[pl.ds(0, root_pieces), 0], part_send)
                wait_for(stats.at[pl.ds(0, NQB), 0], stat_send)

            @pl.when(is_root_chip)
            def _():
                for _ in range(2):
                    wait_for(root_out, out_send)

            @pl.when(is_x_chip)
            def _():
                for _ in range(2):
                    wait_for(x_bf, x_send)

            @pl.when(is_q_chip)
            def _():
                wait_for(root_out.at[:, 0], out_send)
                for _ in range(3):
                    wait_for(q_bf.at[:, 0], q_send)

    dma = pltpu.SemaphoreType.DMA

    def fn(x, Wq, K_ext, V_ext, Wo):
        out = pl.pallas_call(
            body,
            out_shape=jax.ShapeDtypeStruct((SQ, DM), BF16),
            in_specs=[pl.BlockSpec(memory_space=pltpu.HBM)] * 5,
            out_specs=pl.BlockSpec(memory_space=pltpu.VMEM),
            scratch_shapes=[
                pltpu.VMEM((NPIECE, KBLKS, BLK, DH), F32),
                pltpu.VMEM((NPIECE, KBLKS, BLK, DH), F32),
                pltpu.VMEM((NQB, BLK, DM), F32),
                pltpu.VMEM((DM, DM // 2), F32),
                pltpu.VMEM((DM, DM), F32),
                pltpu.VMEM((NQB, BLK, DM), BF16),
                pltpu.VMEM((DM, DM // 2), BF16),
                pltpu.VMEM((NQB, 2, HEADS // 2, BLK, DH), BF16),
                pltpu.VMEM((NPIECE, 4, BLK, DH), BF16),
                pltpu.VMEM((n_group, 4, 8, DH), F32),
                pltpu.VMEM((n_mid, SQ, DH), BF16),
                pltpu.VMEM((NQB, 2, BLK // 2, DM), BF16),
                pltpu.VMEM((SQ, DM), F32),
                dma((NPIECE,)), dma((NPIECE,)), dma((NQB,)), dma((3,)),
                dma((NQB,)), dma((NQB,)), dma((n_group,)), dma((n_group,)), dma((NQB,)),
                dma, dma, dma, dma, dma,
            ],
            compiler_params=pltpu.CompilerParams(
                collective_id=0,
                vmem_limit_bytes=64 << 20,
                disable_bounds_checks=not checks,
                disable_semaphore_checks=not checks,
            ),
        )(
            x.reshape(NQB, BLK, DM),
            Wq,
            K_ext.reshape(KBLKS, NQB, BLK, HEADS, DH),
            V_ext.reshape(KBLKS, NQB, BLK, HEADS, DH),
            Wo,
        )
        return out.reshape(1, SQ, DM)

    return fn


def pallas_dist_sparse_attn_strided_kvseq_b1_sq256_skv4096_hq8_dh128_kernel(x, Wq, K_ext, V_ext, Wo):
    return make()(x, Wq, K_ext, V_ext, Wo)
```

```python
import contextlib
import math

import jax
import jax.numpy as jnp
from jax import lax
from jax.experimental import pallas as pl
from jax.experimental.pallas import tpu as pltpu

SQ, DM, HEADS, DH = 256, 1024, 8, 128
BLK = 64
NQB = SQ // BLK
KBLKS = 16
NPIECE = NQB * HEADS
LAST = NPIECE - 1
LOG2E = math.log2(math.e)
Q_SCALE = 0.08838834764831843 * LOG2E
F32, BF16 = jnp.float32, jnp.bfloat16
MESH = pl.DeviceIdType.MESH


def make(n_root=5, first_piece=17, lag=5, end_tick=63, pull=62, x0=0, perm=([2, 15, 1, 14, 12, 0, 11, 8, 10, 7, 3, 6, 4, 13, 9, 5, 0, 9, 13, 8, 14, 7, 5, 15, 6, 2, 3, 12, 10, 11, 4, 1], [0, 0, 0, 0, 0, 0, 0, 0, 0, 0, 1, 0, 0, 0, 0, 0]), x_at=(0, 2, 3, 4), q_at=(7, 11, 19, 24),
         root_at=(30, 36, 40, 46), fwd_at=(40, 46, 52, 58), take_at=(48, 54, 60, 63), mid_at=(54, 61),
         sizes=(40, 24), mul=3, scope=False, checks=False, pre=4, halves=2, split=(8, 8), trail=2, wq_rows=16, wo_rows=8, wq_mul=1, wo_mul=33):
    n_mid = HEADS - 1 - n_root
    root_pieces = NQB * n_root
    tail_piece = NPIECE - NQB
    tail_group = NQB + n_mid
    n_group = tail_group + 1

    def sc(name):
        return jax.named_scope("s_" + name) if scope else contextlib.nullcontext()

    def body(x_hbm, wq_hbm, k_hbm, v_hbm, wo_hbm, out_ref,
             kbuf, vbuf, x_f32, wq_f32, wo_f32, x_bf, q_bf,
             part, stats, last_stat, root_out, acc, lse_rows, last_acc,
             k_sem, v_sem, w_sem, wo_sem,
             x_recv, q_recv, part_recv, stat_recv, out_recv,
             x_send, q_send, part_send, stat_send, out_send, last_send):

        def coords(p):
            if isinstance(p, int):
                return divmod(p, n_root) if p < root_pieces else ((p - root_pieces) % NQB, n_root + (p - root_pieces) // NQB)
            r = p - root_pieces
            is_root = p < root_pieces
            return (jnp.where(is_root, lax.div(p, n_root), r & (NQB - 1)),
                    jnp.where(is_root, lax.rem(p, n_root), n_root + (r >> 2)))

        chunks = [(i * mul % KBLKS, sum(sizes[:k]), n) for k, n in enumerate(sizes) for i in range(KBLKS)]

        if perm:
            chunks = [(g, (24 if perm[1][g] else 0), 40) for g in perm[0][:16]] + [(g, (0 if perm[1][g] else 40), 24) for g in perm[0][16:]]

        def fetch(src, dst, sem, p, lo=0, hi=len(chunks)):
            b, h = coords(p)
            for i in range(lo, hi):
                g, r0, n = chunks[i]
                rows = pl.ds(r0, n)
                pltpu.make_async_copy(src.at[g, b, rows, h, :], dst.at[p, g, rows], sem.at[p]).start(priority=i % 2)

        spans = [(sum(split[:i]), n) for i, n in enumerate(split)]

        def fetch_in_order(src, dst, sem, g0, n):
            b, h = coords(LAST)

            @pl.loop(g0, g0 + n)
            def _(g):
                pltpu.make_async_copy(src.at[g, b, :, h, :], dst.at[LAST, g], sem).start(priority=1)

        def wo_copy(r):
            rows = pl.ds((n_root + r) * DH, DH)
            return pltpu.make_async_copy(wo_hbm.at[rows], wo_f32.at[rows], wo_sem.at[r])

        def wo_last(i):
            idx = (pl.ds(DM - DH, DH), pl.ds(i * (DM // halves), DM // halves))
            return pltpu.make_async_copy(wo_hbm.at[idx], wo_f32.at[idx], wo_sem.at[n_mid + i])

        def wait_for(ref, sem):
            pltpu.make_async_copy(ref, ref, sem).wait()

        def send(src, dst, send_sem, recv_sem, peer):
            pltpu.make_async_remote_copy(src, dst, send_sem, recv_sem, device_id=(peer,),
                                         device_id_type=MESH).start()

        fetch(k_hbm, kbuf, k_sem, 0, 0, pre)
        me = lax.axis_index("i")
        is_root_chip = me == 0
        not_root_chip = me != 0
        is_x_chip = me == 2
        is_q_chip = (me & 1) == 1
        half = me >> 1
        hop0 = jnp.where(is_root_chip, 2, me)
        hop1 = jnp.where(hop0 == 3, 1, hop0 + 1)
        hop2 = 6 - hop0 - hop1

        @pl.when(is_q_chip)
        def _():
            cols = pl.ds(pl.multiple_of(half * (DM // 2), DM // 2), DM // 2)
            n = DM // wq_rows

            @pl.loop(0, n // 2)
            def _(c):
                for pr in (0, 1):
                    rows = pl.ds(pl.multiple_of((((2 * c + pr) * wq_mul) & (n - 1)) * wq_rows, wq_rows), wq_rows)
                    pltpu.make_async_copy(wq_hbm.at[rows, cols], wq_f32.at[rows], w_sem.at[0]).start(priority=pr)

        @pl.when(is_root_chip)
        def _():
            if x0:
                pltpu.make_async_copy(x_hbm.at[0, pl.ds(0, x0)], x_f32.at[0, pl.ds(0, x0)], w_sem.at[1]).start()
            n = (HEADS - 1) * DH // wo_rows

            @pl.loop(0, n // 2)
            def _(c):
                for pr in (0, 1):
                    i = lax.rem((2 * c + pr) * wo_mul, n)
                    rows = pl.ds(pl.multiple_of(i * wo_rows, wo_rows), wo_rows)
                    pltpu.make_async_copy(wo_hbm.at[rows], wo_f32.at[rows], w_sem.at[0]).start(priority=pr)

        @pl.when(is_x_chip)
        def _():
            @pl.loop(0, SQ // 16)
            def _(c):
                for pr in (0, 1):
                    b = (c >> 3) * 2 + pr
                    rows = pl.ds(pl.multiple_of((c & 7) * 8, 8), 8)
                    cp = pltpu.make_async_copy(x_hbm.at[b, rows], x_f32.at[b, rows], w_sem.at[b])
                    if pr == 0 and x0:
                        pl.when(c >= x0 // 8)(lambda: cp.start(priority=0))
                    else:
                        cp.start(priority=pr)

        barrier = pltpu.get_barrier_semaphore()
        for j in (1, 2, 3):
            pl.semaphore_signal(barrier, inc=1, device_id=(me ^ j,), device_id_type=MESH)
        lse_rows[...] = jnp.zeros((8, DH), F32)

        def on_diagonal():
            lane = lax.broadcasted_iota(jnp.int32, (BLK, DH), 1)
            return (lane & (BLK - 1)) == lax.broadcasted_iota(jnp.int32, (BLK, DH), 0)

        def send_x_rows(b, r0, n, sem):
            rows = pl.ds(r0, n)
            wait_for(x_f32.at[b, rows], sem)
            x_bf[b, rows, :] = x_f32[b, rows, :].astype(BF16)
            for j in (1, 3):
                send(x_bf.at[b, rows], x_bf.at[b, rows], x_send, x_recv.at[b], j)

        def send_x(b):
            if x0:
                pl.when(b == 0)(lambda: send_x_rows(0, x0, BLK - x0, w_sem.at[0]))
                pl.when(b > 0)(lambda: send_x_rows(b, 0, BLK, w_sem.at[b]))
            else:
                send_x_rows(b, 0, BLK, w_sem.at[b])

        def project_q(b):
            @pl.when(b == 0)
            def _():
                wait_for(wq_f32, w_sem.at[0])
            wait_for(x_bf.at[b], x_recv.at[b])
            q = jnp.dot(x_bf[b], wq_f32[...].astype(BF16), preferred_element_type=F32) * Q_SCALE
            q = q.astype(BF16)
            for i in range(HEADS // 2):
                q_bf[b, half, i] = q[:, i * DH:(i + 1) * DH]
            for j in (2, 1, 3):
                send(q_bf.at[b, half], q_bf.at[b, half], q_send, q_recv.at[b], me ^ j)

        def mix_weights(lse):
            top = jnp.maximum(jnp.maximum(lse[0], lse[1]), jnp.maximum(lse[2], lse[3]))
            e = [jnp.exp2(s - top) for s in lse]
            inv = 1.0 / ((e[0] + e[1]) + (e[2] + e[3]))
            low = lax.broadcasted_iota(jnp.int32, top.shape, 1) < BLK
            return [jnp.where(low, e[j], e[j + 1]) * inv for j in (0, 2)]

        def merge_group(g, p0, n):
            wait_for(stats.at[g, pl.ds(1, 3)], stat_recv.at[g])
            wait_for(part.at[pl.ds(p0, n), pl.ds(1, 3)], part_recv.at[g])
            pairs = mix_weights([stats[g, j] for j in range(4)])
            diag = on_diagonal()
            merged = []
            for i in range(n):
                mix = jnp.concatenate([jnp.where(diag, w[i:i + 1], 0.0) for w in pairs], axis=1).astype(BF16)
                merged.append(jnp.dot(mix, part[p0 + i].reshape(4 * BLK, DH), preferred_element_type=F32).astype(BF16))
            return merged

        def project_root(b):
            @pl.when(b == 0)
            def _():
                wait_for(wo_f32.at[pl.ds(0, (HEADS - 1) * DH)], w_sem.at[0])
            c = jnp.concatenate(merge_group(b, b * n_root, n_root), axis=1)
            res = jnp.dot(c, wo_f32[pl.ds(0, n_root * DH), :].astype(BF16), preferred_element_type=F32)
            acc[pl.ds(pl.multiple_of(b * BLK, BLK), BLK), :] = res
            root_out[b] = res.astype(BF16).reshape(2, BLK // 2, DM)
            for j in (1, 3):
                send(root_out.at[b], root_out.at[b], out_send, out_recv.at[b], j)

        def take_root(b):
            wait_for(root_out.at[b], out_recv.at[b])

            @pl.when(is_q_chip)
            def _():
                send(root_out.at[b, half], root_out.at[b, half], out_send, out_recv.at[b], 2)
            acc[pl.ds(pl.multiple_of(b * BLK, BLK), BLK), :] = root_out[b].reshape(BLK, DM).astype(F32)

        def project_mid(r):
            c = jnp.concatenate(merge_group(NQB + r, root_pieces + r * NQB, NQB), axis=0)
            rows = pl.ds(pl.multiple_of((n_root + r) * DH, DH), DH)

            @pl.when(not_root_chip)
            def _():
                wait_for(wo_f32.at[rows], wo_sem.at[r])
            acc[...] += jnp.dot(c, wo_f32[rows, :].astype(BF16), preferred_element_type=F32)

        def scores(k, b, h):
            q = q_bf[b, h >> 2, h & 3]
            s = lax.dot_general(q, k.astype(BF16), (((1,), (1,)), ((), ())), preferred_element_type=F32)
            m = jnp.max(s, axis=1, keepdims=True)
            e = jnp.exp2(s - m)
            l = jnp.sum(e, axis=1, keepdims=True)
            row = jnp.sum(jnp.where(on_diagonal(), m + jnp.log(l) * LOG2E, 0.0), axis=0, keepdims=True)
            return e.astype(BF16), 1.0 / l, row

        def piece(p):
            b, h = coords(p)
            is_root = p < root_pieces
            g = jnp.where(is_root, b, h + (NQB - n_root))
            slot = jnp.where(is_root, h, b)

            @pl.when(jnp.logical_and(h == 0, is_q_chip))
            def _():
                wait_for(q_bf.at[b, 1 - half], q_recv.at[b])

            @pl.when(jnp.logical_and(h == 0, jnp.logical_not(is_q_chip)))
            def _():
                wait_for(q_bf.at[b], q_recv.at[b])

            def share(buf, i, send_sem, recv_sem):
                @pl.when(jnp.logical_or(not_root_chip, jnp.logical_not(is_root)))
                def _():
                    send(buf.at[i, 0], buf.at[i, hop0], send_sem, recv_sem.at[g], me ^ hop0)

                @pl.when(jnp.logical_not(is_root))
                def _():
                    for j in (hop1, hop2):
                        send(buf.at[i, 0], buf.at[i, j], send_sem, recv_sem.at[g], me ^ j)

            wait_for(kbuf.at[p], k_sem.at[p])
            wait_for(vbuf.at[p], v_sem.at[p])
            e, inv, row = scores(kbuf[p].reshape(KBLKS * BLK, DH), b, h)
            rows = jnp.where(lax.broadcasted_iota(jnp.int32, (8, DH), 0) == slot, row, lse_rows[...])
            lse_rows[...] = rows
            v = vbuf[p].reshape(KBLKS * BLK, DH).astype(BF16)
            part[p, 0] = (jnp.dot(e, v, preferred_element_type=F32) * inv).astype(BF16)

            @pl.when(jnp.logical_or(slot == jnp.where(is_root, n_root - 1, NQB - 1), p == LAST - 1))
            def _():
                stats[g, 0] = rows
                share(stats, g, stat_send, stat_recv)

            share(part, p, part_send, part_recv)

        def fetch_trailing():
            @pl.when(not_root_chip)
            def _():
                for r in range(n_mid):
                    wo_copy(r).start(priority=1)
                for i in range(halves):
                    wo_last(i).start(priority=1)

        def last_piece():
            b, h = coords(LAST)
            wait_for(kbuf.at[LAST], k_sem.at[LAST])
            e, inv, row = scores(kbuf[LAST].reshape(KBLKS * BLK, DH), b, h)
            last_stat[0] = row
            for j in (hop0, hop1, hop2):
                send(last_stat.at[0], last_stat.at[j], stat_send, stat_recv.at[n_group], me ^ j)
            o = None
            for i, (g0, n) in enumerate(spans):
                wait_for(vbuf.at[LAST, pl.ds(g0, n)], v_sem.at[LAST + i])
                if trail == i + 1:
                    fetch_trailing()
                v = vbuf[LAST, pl.ds(g0, n)].reshape(n * BLK, DH).astype(BF16)
                t = jnp.dot(e[:, g0 * BLK:(g0 + n) * BLK], v, preferred_element_type=F32)
                o = t if o is None else last_acc[...] + t
                if i + 1 < len(spans):
                    last_acc[...] = o
            part[LAST, 0] = (o * inv).astype(BF16)
            for j in (hop0, hop1, hop2):
                send(part.at[LAST, 0], part.at[LAST, j], last_send, part_recv.at[n_group], me ^ j)
            if trail == -1:
                fetch_trailing()

        def tick(j, p):
            with sc("issue"):
                @pl.when(jnp.logical_and((j & 1) == 0, j < 2 * LAST))
                def _():
                    if pre:
                        pl.when(j > 0)(lambda: fetch(k_hbm, kbuf, k_sem, j >> 1, 0, pre))
                    fetch(k_hbm, kbuf, k_sem, j >> 1, pre)

                @pl.when(jnp.logical_and((j & 1) == 1, j < 2 * LAST))
                def _():
                    fetch(v_hbm, vbuf, v_sem, j >> 1)

                @pl.when(j == 2 * LAST)
                def _():
                    fetch_in_order(k_hbm, kbuf, k_sem.at[LAST], 0, KBLKS)
                    for i, (g0, n) in enumerate(spans):
                        fetch_in_order(v_hbm, vbuf, v_sem.at[LAST + i], g0, n)

                    @pl.when(is_root_chip)
                    def _():
                        for i in range(halves):
                            wo_last(i).start(priority=1)
                    if trail == 0:
                        fetch_trailing()

            @pl.when(j == 0)
            def _():
                pl.semaphore_wait(barrier, 3)
                if x0:
                    pl.when(is_root_chip)(lambda: send_x_rows(0, 0, x0, w_sem.at[1]))

            def task(name, on_chip, ticks, f):
                which = sum(jnp.where(j == at, i + 1, 0) for i, at in enumerate(ticks))
                run = jnp.logical_and(on_chip, which > 0)

                @pl.when(run)
                def _():
                    with sc(name):
                        f(which - 1)
                return run

            task("x", is_x_chip, x_at, send_x)
            busy = task("q", is_q_chip, q_at, project_q)
            busy |= task("root", is_root_chip, root_at, project_root)
            run = (j >= first_piece) & (j >= jnp.minimum(2 * p + lag, pull)) & (p < LAST) & jnp.logical_not(busy)

            @pl.when(run)
            def _():
                with sc("piece"):
                    piece(p)

            @pl.when(j == end_tick)
            def _():
                with sc("last"):
                    last_piece()

            task("take", not_root_chip, [jnp.where(is_x_chip, a, c) for a, c in zip(take_at, fwd_at)], take_root)
            which = sum(jnp.where(j == at, i + 1, 0) for i, at in enumerate(mid_at))
            hi = jnp.where(is_root_chip, which, jnp.where(j == end_tick, n_mid, 0))

            @pl.loop(jnp.where(is_root_chip, jnp.maximum(which - 1, 0), 0), hi)
            def _(r):
                with sc("mid"):
                    project_mid(r)
            return p + run.astype(jnp.int32)

        lax.fori_loop(0, end_tick + 1, tick, jnp.int32(0))

        top, bottom = pl.ds(0, SQ - BLK), pl.ds(SQ - BLK, BLK)
        with sc("merge7"):
            head = jnp.concatenate(merge_group(tail_group, tail_piece, NQB - 1), axis=0)


        @pl.when(not_root_chip)
        def _():
            wait_for(part.at[pl.ds(0, root_pieces), 0], part_send)
            wait_for(stats.at[pl.ds(0, NQB), 0], stat_send)

        @pl.when(is_root_chip)
        def _():
            for _ in range(2):
                wait_for(root_out, out_send)
                if x0:
                    wait_for(x_bf.at[0, pl.ds(0, x0)], x_send)

        @pl.when(is_x_chip)
        def _():
            for _ in range(2):
                wait_for(x_bf.at[0, pl.ds(x0, BLK - x0)], x_send)
                wait_for(x_bf.at[pl.ds(1, 3)], x_send)

        @pl.when(is_q_chip)
        def _():
            wait_for(root_out.at[:, 0], out_send)
            for _ in range(3):
                wait_for(q_bf.at[:, 0], q_send)

        wo = []
        for i in range(halves):
            with sc("top"):
                wo_last(i).wait()
                if i == halves - 1:
                    wait_for(last_stat.at[pl.ds(1, 3)], stat_recv.at[n_group])
                    w = [jnp.broadcast_to(pair, (DH, DH)).T for pair in mix_weights([last_stat[j] for j in range(4)])]
                cols = pl.ds(i * (DM // halves), DM // halves)
                wo.append(wo_f32[pl.ds(DM - DH, DH), cols].astype(BF16))
                out_ref[top, cols] = (acc[top, cols] + jnp.dot(head, wo[i], preferred_element_type=F32)).astype(BF16)
        wo = jnp.concatenate(wo, axis=1)
        wait_for(part.at[pl.ds(root_pieces, LAST - root_pieces), pl.ds(1, 3)], part_send)
        wait_for(stats.at[pl.ds(NQB, n_group - NQB), pl.ds(1, 3)], stat_send)
        wait_for(last_stat.at[pl.ds(1, 3)], stat_send)
        with sc("final"):
            wait_for(part.at[LAST, pl.ds(1, 3)], part_recv.at[n_group])
            t = [part[LAST, j].astype(F32) * w[j // 2][(j % 2) * BLK:(j % 2 + 1) * BLK] for j in range(4)]
            tail = ((t[0] + t[1]) + (t[2] + t[3])).astype(BF16)
            out_ref[bottom, :] = (acc[bottom, :] + jnp.dot(tail, wo, preferred_element_type=F32)).astype(BF16)
        wait_for(part.at[LAST, pl.ds(1, 3)], last_send)

    def piece_ticks(busy):
        out, p = [], 0
        for j in range(end_tick + 1):
            if j >= first_piece and j >= min(2 * p + lag, pull) and p < LAST and j not in busy:
                out.append(j)
                p += 1
        return out

    plans = [piece_ticks(set(root_at)), piece_ticks(set(q_at)), piece_ticks(set())]
    assert all(len(t) == LAST for t in plans)
    for b in range(NQB):
        assert x_at[b] < q_at[b] < min(t[b * n_root] for t in plans)
        assert max(t[(b + 1) * n_root - 1] for t in plans) < root_at[b] < fwd_at[b] < take_at[b] <= end_tick
    for r in range(n_mid):
        assert max(root_at[-1], max(t[root_pieces + (r + 1) * NQB - 1] for t in plans)) <= mid_at[r] <= end_tick

    dma = pltpu.SemaphoreType.DMA

    def fn(x, Wq, K_ext, V_ext, Wo):
        out = pl.pallas_call(
            body,
            out_shape=jax.ShapeDtypeStruct((SQ, DM), BF16),
            in_specs=[pl.BlockSpec(memory_space=pltpu.HBM)] * 5,
            out_specs=pl.BlockSpec(memory_space=pltpu.VMEM),
            scratch_shapes=[
                pltpu.VMEM((NPIECE, KBLKS, BLK, DH), F32),
                pltpu.VMEM((NPIECE, KBLKS, BLK, DH), F32),
                pltpu.VMEM((NQB, BLK, DM), F32),
                pltpu.VMEM((DM, DM // 2), F32),
                pltpu.VMEM((DM, DM), F32),
                pltpu.VMEM((NQB, BLK, DM), BF16),
                pltpu.VMEM((NQB, 2, HEADS // 2, BLK, DH), BF16),
                pltpu.VMEM((NPIECE, 4, BLK, DH), BF16),
                pltpu.VMEM((n_group, 4, 8, DH), F32),
                pltpu.VMEM((4, 1, DH), F32),
                pltpu.VMEM((NQB, 2, BLK // 2, DM), BF16),
                pltpu.VMEM((SQ, DM), F32),
                pltpu.VMEM((8, DH), F32),
                pltpu.VMEM((BLK, DH), F32),
                dma((NPIECE,)), dma((LAST + len(split),)), dma((NQB,)), dma((n_mid + halves,)),
                dma((NQB,)), dma((NQB,)), dma((n_group + 1,)), dma((n_group + 1,)), dma((NQB,)),
                dma, dma, dma, dma, dma, dma,
            ],
            compiler_params=pltpu.CompilerParams(
                collective_id=0,
                vmem_limit_bytes=64 << 20,
                disable_bounds_checks=not checks,
                disable_semaphore_checks=not checks,
            ),
        )(
            x.reshape(NQB, BLK, DM),
            Wq,
            K_ext.reshape(KBLKS, NQB, BLK, HEADS, DH),
            V_ext.reshape(KBLKS, NQB, BLK, HEADS, DH),
            Wo,
        )
        return out.reshape(1, SQ, DM)

    return fn


def pallas_dist_sparse_attn_strided_kvseq_b1_sq256_skv4096_hq8_dh128_kernel(x, Wq, K_ext, V_ext, Wo):
    return make()(x, Wq, K_ext, V_ext, Wo)
```

```python
import math

import jax
import jax.numpy as jnp
from jax import lax
from jax.experimental import pallas as pl
from jax.experimental.pallas import tpu as pltpu

F32, BF16 = jnp.float32, jnp.bfloat16
MESH = pl.DeviceIdType.MESH

N_DEV = 4
SQ, DM, HEADS, DH = 256, 1024, 8, 128
BLK = 64
NQB = SQ // BLK
KBLKS = 16
LOG2E = math.log2(math.e)
Q_SCALE = 0.08838834764831843 * LOG2E

ROOT_HEADS = 5
MID_HEADS = HEADS - 1 - ROOT_HEADS
N_PIECE = NQB * HEADS
ROOT_PIECES = NQB * ROOT_HEADS
TAIL_PIECE = N_PIECE - NQB
LAST = N_PIECE - 1

TAIL_GROUP = NQB + MID_HEADS
LAST_GROUP = TAIL_GROUP + 1
N_GROUP = LAST_GROUP + 1

PASSES = ((0, 40), (40, 24))
K_ORDER = (
    (9, 13, 10, 14, 12, 1, 15, 7, 11, 8, 4, 0, 3, 5, 2, 6),
    (9, 1, 5, 8, 10, 7, 12, 0, 11, 15, 3, 14, 2, 6, 4, 13),
)
V_ORDER = (
    (12, 15, 2, 0, 1, 14, 11, 8, 3, 6, 10, 7, 4, 5, 9, 13),
    (11, 9, 13, 8, 6, 7, 5, 0, 4, 1, 3, 2, 14, 12, 15, 10),
)
HEAD_START = 4
WQ_STRIDE = 9
WO_STRIDE = 11

LAST_FETCH = 2 * LAST
END_TICK = LAST_FETCH + 1
FIRST_PIECE_AT = 17
PIECE_LAG = 5
SEND_X_AT = (0, 2, 3, 4)
PROJECT_Q_AT = (7, 11, 19, 24)
PROJECT_ROOT_AT = (30, 36, 42, 46)
FORWARD_ROOT_AT = (42, 48, 54, 58)
TAKE_ROOT_AT = (50, 56, 62, END_TICK)
PROJECT_MID_AT = (56, 61)
DRAIN_AT = 58


def _coords(p):
    r = p - ROOT_PIECES
    if isinstance(p, int):
        return divmod(p, ROOT_HEADS) if r < 0 else (r % NQB, ROOT_HEADS + r // NQB)
    return (
        jnp.where(r < 0, lax.div(p, ROOT_HEADS), r & (NQB - 1)),
        jnp.where(r < 0, lax.rem(p, ROOT_HEADS), ROOT_HEADS + (r >> 2)),
    )


def _wait(ref, sem):
    pltpu.make_async_copy(ref, ref, sem).wait()


def _send(src, dst, send_sem, recv_sem, peer):
    pltpu.make_async_remote_copy(
        src, dst, send_sem, recv_sem, device_id=(peer,), device_id_type=MESH
    ).start()


def _dot(a, b):
    return jnp.dot(a, b, preferred_element_type=F32)


def _on_diagonal():
    lane = lax.broadcasted_iota(jnp.int32, (BLK, DH), 1)
    return (lane & (BLK - 1)) == lax.broadcasted_iota(jnp.int32, (BLK, DH), 0)


def _chip_weights(lse):
    top = jnp.maximum(jnp.maximum(lse[0], lse[1]), jnp.maximum(lse[2], lse[3]))
    e = [jnp.exp2(s - top) for s in lse]
    inv = 1.0 / ((e[0] + e[1]) + (e[2] + e[3]))
    low = lax.broadcasted_iota(jnp.int32, top.shape, 1) < BLK
    return [jnp.where(low, e[j], e[j + 1]) * inv for j in (0, 2)]


def _kernel(
    x_hbm, wq_hbm, k_hbm, v_hbm, wo_hbm,
    out_ref,
    k_buf, v_buf, x_f32, wq_f32, wo_f32, x_bf, q_bf,
    part, stats, root_out, acc, lse_rows, last_acc,
    k_sem, v_sem, w_sem, wo_sem,
    x_recv, q_recv, part_recv, stat_recv, out_recv,
    x_send, q_send, part_send, stat_send, out_send,
):
    def fetch(src, dst, sem, order, p, lo=0, hi=len(PASSES) * KBLKS):
        b, h = _coords(p)
        for i in range(lo, hi):
            g = order[i // KBLKS][i % KBLKS]
            keys = pl.ds(*PASSES[i // KBLKS])
            pltpu.make_async_copy(
                src.at[g, b, keys, h, :], dst.at[p, g, keys], sem.at[p]
            ).start(priority=i % 2)

    def fetch_last(src, dst, sem, first, count):
        b, h = _coords(LAST)

        @pl.loop(first, first + count)
        def _(g):
            pltpu.make_async_copy(
                src.at[g, b, :, h, :], dst.at[LAST, g], sem
            ).start(priority=1)

    def wo_mid_copy(r):
        rows = pl.ds((ROOT_HEADS + r) * DH, DH)
        return pltpu.make_async_copy(wo_hbm.at[rows], wo_f32.at[rows], wo_sem.at[r])

    def wo_last_copy(side):
        idx = (pl.ds(DM - DH, DH), pl.ds(side * (DM // 2), DM // 2))
        return pltpu.make_async_copy(
            wo_hbm.at[idx], wo_f32.at[idx], wo_sem.at[MID_HEADS + side]
        )

    fetch(k_hbm, k_buf, k_sem, K_ORDER, 0, 0, HEAD_START)

    me = lax.axis_index("i")
    is_root_chip = me == 0
    not_root_chip = me != 0
    is_x_chip = me == 2
    is_q_chip = (me & 1) == 1
    half = me >> 1
    hop0 = jnp.where(is_root_chip, 2, me)
    hop1 = jnp.where(hop0 == 3, 1, hop0 + 1)
    hops = (hop0, hop1, 6 - hop0 - hop1)

    barrier = pltpu.get_barrier_semaphore()
    for j in range(1, N_DEV):
        pl.semaphore_signal(barrier, inc=1, device_id=(me ^ j,), device_id_type=MESH)

    def fetch_weight(src, cols, dst, n_rows, stride):
        tiles = n_rows // 8

        def pair(_, tile):
            for prio in (0, 1):
                rows = pl.ds(pl.multiple_of(tile * 8, 8), 8)
                pltpu.make_async_copy(
                    src.at[rows, cols], dst.at[rows], w_sem.at[0]
                ).start(priority=prio)
                tile = jnp.where(tile < tiles - stride, tile + stride, tile + stride - tiles)
            return tile

        lax.fori_loop(0, tiles // 2, pair, jnp.int32(0))

    @pl.when(is_q_chip)
    def _():
        cols = pl.ds(pl.multiple_of(half * (DM // 2), DM // 2), DM // 2)
        fetch_weight(wq_hbm, cols, wq_f32, DM, WQ_STRIDE)

    @pl.when(is_root_chip)
    def _():
        fetch_weight(wo_hbm, slice(None), wo_f32, DM - DH, WO_STRIDE)

    @pl.when(is_x_chip)
    def _():
        @pl.loop(0, SQ // 16)
        def _(c):
            for prio in (0, 1):
                b = (c >> 3) * 2 + prio
                rows = pl.ds(pl.multiple_of((c & 7) * 8, 8), 8)
                pltpu.make_async_copy(
                    x_hbm.at[b, rows], x_f32.at[b, rows], w_sem.at[b]
                ).start(priority=prio)

    lse_rows[...] = jnp.zeros((8, DH), F32)

    def drain(ref, sem):
        pltpu.make_async_remote_copy(
            ref, ref, sem, sem, device_id=(me,), device_id_type=MESH
        ).wait_send()

    def drain_early_sends():
        @pl.loop(0, jnp.where(is_root_chip, 2, 0))
        def _(i):
            drain(root_out, out_send.at[i])

        @pl.loop(0, jnp.where(is_x_chip, 2, 0))
        def _(i):
            drain(x_bf, x_send.at[i])

        @pl.loop(0, jnp.where(is_q_chip, 3, 0))
        def _(i):
            drain(q_bf.at[:, half], q_send.at[i])

        @pl.when(not_root_chip)
        def _():
            drain(part.at[pl.ds(0, ROOT_PIECES), 0], part_send.at[0])
            drain(stats.at[pl.ds(0, NQB), 0], stat_send.at[0])

    def send_x(b):
        _wait(x_f32.at[b], w_sem.at[b])
        x_bf[b] = x_f32[b].astype(BF16)
        for i, peer in enumerate((1, 3)):
            _send(x_bf.at[b], x_bf.at[b], x_send.at[i], x_recv.at[b], peer)

    def project_q(b):
        pl.when(b == 0)(lambda: _wait(wq_f32, w_sem.at[0]))
        _wait(x_bf.at[b], x_recv.at[b])
        q = (_dot(x_bf[b], wq_f32[...].astype(BF16)) * Q_SCALE).astype(BF16)
        for i in range(HEADS // 2):
            q_bf[b, half, i] = q[:, i * DH:(i + 1) * DH]
        for i, j in enumerate((2, 1, 3)):
            _send(
                q_bf.at[b, half], q_bf.at[b, half],
                q_send.at[i], q_recv.at[2 * b + half], me ^ j,
            )

    def softmax(p, b, h):
        k = k_buf[p].reshape(KBLKS * BLK, DH).astype(BF16)
        s = lax.dot_general(
            q_bf[b, h >> 2, h & 3], k, (((1,), (1,)), ((), ())), preferred_element_type=F32
        )
        m = jnp.max(s, axis=1, keepdims=True)
        e = jnp.exp2(s - m)
        total = jnp.sum(e, axis=1, keepdims=True)
        lse = jnp.where(_on_diagonal(), m + jnp.log(total) * LOG2E, 0.0)
        return e.astype(BF16), 1.0 / total, jnp.sum(lse, axis=0, keepdims=True)

    def piece(p):
        b, h = _coords(p)
        to_all = p >= ROOT_PIECES
        group = jnp.where(to_all, h + (NQB - ROOT_HEADS), b)
        slot = jnp.where(to_all, b, h)

        @pl.loop(0, jnp.where(h == 0, jnp.where(is_q_chip, 1, 2), 0))
        def _(i):
            side = (1 - half) ^ i
            _wait(q_bf.at[b, side], q_recv.at[2 * b + side])

        def share(buf, i, send_sem, recv_sem):
            def to(j, sem):
                _send(buf.at[i, 0], buf.at[i, j], send_sem.at[sem], recv_sem.at[group], me ^ j)

            pl.when(jnp.logical_and(not_root_chip, jnp.logical_not(to_all)))(lambda: to(hop0, 0))

            @pl.when(to_all)
            def _():
                for j in hops:
                    to(j, 1)

        _wait(k_buf.at[p], k_sem.at[p])
        _wait(v_buf.at[p], v_sem.at[p])
        e, inv, row = softmax(p, b, h)
        sublane = lax.broadcasted_iota(jnp.int32, (8, DH), 0)
        rows = jnp.where(sublane == slot, row, lse_rows[...])
        lse_rows[...] = rows
        v = v_buf[p].reshape(KBLKS * BLK, DH).astype(BF16)
        part[p, 0] = (_dot(e, v) * inv).astype(BF16)

        @pl.when(jnp.logical_or(slot == jnp.where(to_all, NQB, ROOT_HEADS) - 1, p == LAST - 1))
        def _():
            stats[group, 0] = rows
            share(stats, group, stat_send, stat_recv)

        share(part, p, part_send, part_recv)

    def last_piece():
        _wait(k_buf.at[LAST], k_sem.at[LAST])
        e, inv, row = softmax(LAST, *_coords(LAST))
        stats[LAST_GROUP, 0] = jnp.broadcast_to(row, (8, DH))
        for j in hops:
            _send(
                stats.at[LAST_GROUP, 0, pl.ds(0, 1)], stats.at[LAST_GROUP, j, pl.ds(0, 1)],
                stat_send.at[2], stat_recv.at[LAST_GROUP], me ^ j,
            )

        def weighted(side):
            n = KBLKS // 2
            v = v_buf[LAST, pl.ds(side * n, n)].reshape(n * BLK, DH).astype(BF16)
            return _dot(e[:, side * n * BLK:(side + 1) * n * BLK], v)

        _wait(v_buf.at[LAST, pl.ds(0, KBLKS // 2)], v_sem.at[LAST])
        last_acc[...] = weighted(0)
        _wait(v_buf.at[LAST, pl.ds(KBLKS // 2, KBLKS // 2)], v_sem.at[LAST + 1])

        @pl.when(not_root_chip)
        def _():
            for r in range(MID_HEADS):
                wo_mid_copy(r).start(priority=1)
            for side in (0, 1):
                wo_last_copy(side).start(priority=1)

        rest = weighted(1)
        part[LAST, 0] = ((last_acc[...] + rest) * inv).astype(BF16)
        for j in hops:
            _send(
                part.at[LAST, 0], part.at[LAST, j],
                part_send.at[1], part_recv.at[LAST_GROUP], me ^ j,
            )
        pl.when(is_q_chip)(lambda: drain(root_out.at[:, half], out_send.at[0]))

    def merge(group, first, count):
        _wait(stats.at[group, pl.ds(1, N_DEV - 1)], stat_recv.at[group])
        _wait(part.at[pl.ds(first, count), pl.ds(1, N_DEV - 1)], part_recv.at[group])
        weights = _chip_weights([stats[group, j] for j in range(N_DEV)])
        diagonal = _on_diagonal()
        merged = []
        for i in range(count):
            mix = [jnp.where(diagonal, w[i:i + 1], 0.0) for w in weights]
            mix = jnp.concatenate(mix, axis=1).astype(BF16)
            merged.append(_dot(mix, part[first + i].reshape(N_DEV * BLK, DH)).astype(BF16))
        return merged

    def project_root(b):
        pl.when(b == 0)(lambda: _wait(wo_f32.at[pl.ds(0, DM - DH)], w_sem.at[0]))
        ctx = jnp.concatenate(merge(b, b * ROOT_HEADS, ROOT_HEADS), axis=1)
        res = _dot(ctx, wo_f32[pl.ds(0, ROOT_HEADS * DH), :].astype(BF16))
        acc[pl.ds(pl.multiple_of(b * BLK, BLK), BLK), :] = res
        root_out[b] = res.astype(BF16).reshape(2, BLK // 2, DM)
        for i, peer in enumerate((1, 3)):
            _send(root_out.at[b], root_out.at[b], out_send.at[i], out_recv.at[b], peer)

    def take_root(b):
        _wait(root_out.at[b], out_recv.at[b])

        @pl.when(is_q_chip)
        def _():
            _send(root_out.at[b, half], root_out.at[b, half], out_send.at[0], out_recv.at[b], 2)

        acc[pl.ds(pl.multiple_of(b * BLK, BLK), BLK), :] = (
            root_out[b].reshape(BLK, DM).astype(F32)
        )

    def project_mid(r):
        ctx = jnp.concatenate(merge(NQB + r, ROOT_PIECES + r * NQB, NQB), axis=0)
        rows = pl.ds(pl.multiple_of((ROOT_HEADS + r) * DH, DH), DH)
        pl.when(not_root_chip)(lambda: _wait(wo_f32.at[rows], wo_sem.at[r]))
        acc[...] += _dot(ctx, wo_f32[rows, :].astype(BF16))

    def tick(t, p):
        @pl.when(jnp.logical_and((t & 1) == 0, t < LAST_FETCH))
        def _():
            pl.when(t > 0)(lambda: fetch(k_hbm, k_buf, k_sem, K_ORDER, t >> 1, 0, HEAD_START))
            fetch(k_hbm, k_buf, k_sem, K_ORDER, t >> 1, HEAD_START)

        @pl.when(jnp.logical_and((t & 1) == 1, t < LAST_FETCH))
        def _():
            fetch(v_hbm, v_buf, v_sem, V_ORDER, t >> 1)

        @pl.when(t == LAST_FETCH)
        def _():
            fetch_last(k_hbm, k_buf, k_sem.at[LAST], 0, KBLKS)
            for side in (0, 1):
                fetch_last(v_hbm, v_buf, v_sem.at[LAST + side], side * (KBLKS // 2), KBLKS // 2)

            @pl.when(is_root_chip)
            def _():
                for side in (0, 1):
                    wo_last_copy(side).start(priority=1)

        pl.when(t == 0)(lambda: pl.semaphore_wait(barrier, N_DEV - 1))
        pl.when(t == DRAIN_AT)(drain_early_sends)

        def due(ticks):
            return sum(jnp.where(t == at, i + 1, 0) for i, at in enumerate(ticks))

        def task(on_chip, ticks, run):
            which = due(ticks)
            active = jnp.logical_and(on_chip, which > 0)
            pl.when(active)(lambda: run(which - 1))
            return active

        task(is_x_chip, SEND_X_AT, send_x)
        busy = task(is_q_chip, PROJECT_Q_AT, project_q)
        busy |= task(is_root_chip, PROJECT_ROOT_AT, project_root)
        ready = t >= jnp.clip(2 * p + PIECE_LAG, FIRST_PIECE_AT, LAST_FETCH)
        run_piece = jnp.logical_and(ready, jnp.logical_not(busy))
        pl.when(run_piece)(lambda: piece(p))
        pl.when(t == END_TICK)(last_piece)

        take_at = [jnp.where(is_x_chip, a, b) for a, b in zip(TAKE_ROOT_AT, FORWARD_ROOT_AT)]
        task(not_root_chip, take_at, take_root)

        mid = due(PROJECT_MID_AT)
        lo = jnp.where(is_root_chip, jnp.maximum(mid - 1, 0), 0)
        hi = jnp.where(is_root_chip, mid, jnp.where(t == END_TICK, MID_HEADS, 0))
        pl.loop(lo, hi)(project_mid)
        return p + run_piece.astype(jnp.int32)

    lax.fori_loop(0, END_TICK + 1, tick, jnp.int32(0))

    top, bottom = pl.ds(0, SQ - BLK), pl.ds(SQ - BLK, BLK)
    ctx = jnp.concatenate(merge(TAIL_GROUP, TAIL_PIECE, NQB - 1), axis=0)

    def project_top(side):
        cols = pl.ds(side * (DM // 2), DM // 2)
        wo = wo_f32[pl.ds(DM - DH, DH), cols].astype(BF16)
        out_ref[top, cols] = (acc[top, cols] + _dot(ctx, wo)).astype(BF16)
        return wo

    wo_last_copy(0).wait()
    wo_left = project_top(0)
    wo_last_copy(1).wait()
    _wait(stats.at[LAST_GROUP, pl.ds(1, N_DEV - 1), pl.ds(0, 1)], stat_recv.at[LAST_GROUP])
    weights = _chip_weights([stats[LAST_GROUP, j, pl.ds(0, 1), :] for j in range(N_DEV)])
    weights = [jnp.broadcast_to(w, (DH, DH)).T for w in weights]
    wo = jnp.concatenate([wo_left, project_top(1)], axis=1)

    drain(stats.at[pl.ds(NQB, LAST_GROUP - NQB), pl.ds(1, N_DEV - 1)], stat_send.at[1])
    drain(stats.at[LAST_GROUP, pl.ds(1, N_DEV - 1), pl.ds(0, 1)], stat_send.at[2])

    _wait(part.at[LAST, pl.ds(1, N_DEV - 1)], part_recv.at[LAST_GROUP])
    terms = [
        part[LAST, j].astype(F32) * weights[j // 2][(j % 2) * BLK:(j % 2 + 1) * BLK]
        for j in range(N_DEV)
    ]
    ctx_last = ((terms[0] + terms[1]) + (terms[2] + terms[3])).astype(BF16)
    out_ref[bottom, :] = (acc[bottom, :] + _dot(ctx_last, wo)).astype(BF16)
    drain(part.at[pl.ds(ROOT_PIECES, N_PIECE - ROOT_PIECES), pl.ds(1, N_DEV - 1)], part_send.at[1])


def pallas_dist_sparse_attn_strided_kvseq_b1_sq256_skv4096_hq8_dh128_kernel(
    x: jax.Array,
    Wq: jax.Array,
    K_ext: jax.Array,
    V_ext: jax.Array,
    Wo: jax.Array,
):
    dma = pltpu.SemaphoreType.DMA
    kv_shape = (KBLKS, NQB, BLK, HEADS, DH)
    out = pl.pallas_call(
        _kernel,
        out_shape=jax.ShapeDtypeStruct((SQ, DM), BF16),
        in_specs=[pl.BlockSpec(memory_space=pltpu.HBM)] * 5,
        out_specs=pl.BlockSpec(memory_space=pltpu.VMEM),
        scratch_shapes=[
            pltpu.VMEM((N_PIECE, KBLKS, BLK, DH), F32),
            pltpu.VMEM((N_PIECE, KBLKS, BLK, DH), F32),
            pltpu.VMEM((NQB, BLK, DM), F32),
            pltpu.VMEM((DM, DM // 2), F32),
            pltpu.VMEM((DM, DM), F32),
            pltpu.VMEM((NQB, BLK, DM), BF16),
            pltpu.VMEM((NQB, 2, HEADS // 2, BLK, DH), BF16),
            pltpu.VMEM((N_PIECE, N_DEV, BLK, DH), BF16),
            pltpu.VMEM((N_GROUP, N_DEV, 8, DH), F32),
            pltpu.VMEM((NQB, 2, BLK // 2, DM), BF16),
            pltpu.VMEM((SQ, DM), F32),
            pltpu.VMEM((8, DH), F32),
            pltpu.VMEM((BLK, DH), F32),
            dma((N_PIECE,)),
            dma((N_PIECE + 1,)),
            dma((NQB,)),
            dma((MID_HEADS + 2,)),
            dma((NQB,)),
            dma((2 * NQB,)),
            dma((N_GROUP,)),
            dma((N_GROUP,)),
            dma((NQB,)),
            dma((2,)),
            dma((3,)),
            dma((2,)),
            dma((3,)),
            dma((2,)),
        ],
        compiler_params=pltpu.CompilerParams(
            collective_id=0,
            vmem_limit_bytes=64 << 20,
            disable_bounds_checks=True,
            disable_semaphore_checks=True,
        ),
    )(x.reshape(NQB, BLK, DM), Wq, K_ext.reshape(kv_shape), V_ext.reshape(kv_shape), Wo)
    return out.reshape(1, SQ, DM)
```
